```python
import numpy as np

kernel_name = "dist_mean_ax0_shard0_i_m4096_n1024"

def setup_inputs():
    return {"x": np.random.randn(16384, 1024).astype(np.float32)}

def reference(x: np.ndarray) -> np.ndarray:
    return np.mean(x, axis=0, keepdims=True)
```

```python
import jax
import jax.numpy as jnp
from jax import lax
from jax.experimental import pallas as pl
from jax.experimental.pallas import tpu as pltpu

NUM_DEVICES = 4
ROWS = 8
STREAMS = 32
LOOKAHEAD = 3
TAIL = (16, 8, 7, 1)


def pallas_dist_mean_ax0_shard0_i_m4096_n1024_kernel(x: jax.Array):
    m, n = x.shape
    per_stream = m // STREAMS
    steps = per_stream // ROWS
    step_rows = STREAMS * ROWS
    assert m == steps * step_rows and steps > LOOKAHEAD and sum(TAIL) == STREAMS

    def kernel_body(x_hbm, o_ref, buf, send_buf, recv_buf, step_sems, tail_sems,
                    send_sems, recv_sems):
        def start_piece(step, stream, sem):
            src = stream * per_stream + step * ROWS
            dst = step * step_rows + stream * ROWS
            if not isinstance(step, int):
                src, dst = pl.multiple_of(src, ROWS), pl.multiple_of(dst, ROWS)
            pltpu.make_async_copy(
                x_hbm.at[pl.ds(src, ROWS)], buf.at[pl.ds(dst, ROWS)], sem
            ).start(priority=stream % 2)

        def start_step(step):
            for stream in range(STREAMS):
                start_piece(step, stream, step_sems.at[step])

        def start_last_step():
            stream = 0
            for t, count in enumerate(TAIL):
                for _ in range(count):
                    start_piece(steps - 1, stream, tail_sems.at[t])
                    stream += 1

        def wait_rows(first, rows, sem):
            block = buf.at[pl.ds(first, rows)]
            pltpu.make_async_copy(block, block, sem).wait()

        def add_rows(first, rows, acc):
            for r in range(0, rows, ROWS):
                acc = acc + buf[pl.ds(first + r, ROWS), :]
            return acc

        def sum_step(step, acc, start_next):
            first = step * step_rows
            if not isinstance(step, int):
                first = pl.multiple_of(first, step_rows)
            wait_rows(first, step_rows, step_sems.at[step])
            start_next()
            return add_rows(first, step_rows, acc)

        for step in range(LOOKAHEAD):
            start_step(step)

        me = lax.axis_index("i")
        barrier = pltpu.get_barrier_semaphore()
        for d in range(1, NUM_DEVICES):
            pl.semaphore_signal(
                barrier, 1, device_id=(me + d) % NUM_DEVICES,
                device_id_type=pl.DeviceIdType.LOGICAL,
            )

        acc = jnp.zeros((ROWS, n), jnp.float32)
        full = steps - 1 - LOOKAHEAD
        acc = lax.fori_loop(
            0, full,
            lambda i, a: sum_step(i, a, lambda: start_step(i + LOOKAHEAD)), acc)
        acc = sum_step(full, acc, start_last_step)
        pl.semaphore_wait(barrier, NUM_DEVICES - 1)
        acc = lax.fori_loop(
            full + 1, steps - 1, lambda i, a: sum_step(i, a, lambda: None), acc)
        first = (steps - 1) * step_rows
        for t, count in enumerate(TAIL):
            wait_rows(first, count * ROWS, tail_sems.at[t])
            acc = add_rows(first, count * ROWS, acc)
            first += count * ROWS

        part = jnp.sum(acc, axis=0, keepdims=True) * (1.0 / (m * NUM_DEVICES))
        send_buf[...] = part

        def exchange(d):
            return pltpu.make_async_remote_copy(
                send_buf, recv_buf.at[d - 1], send_sems.at[d - 1], recv_sems.at[d - 1],
                device_id=(me + d) % NUM_DEVICES,
                device_id_type=pl.DeviceIdType.LOGICAL,
            )

        for d in (2, 1, 3):
            exchange(d).start()
        exchange(1).wait_recv()
        exchange(3).wait_recv()
        neighbours = recv_buf[0] + recv_buf[2]
        for d in (2, 1, 3):
            exchange(d).wait_send()
        exchange(2).wait_recv()
        o_ref[...] = (part + recv_buf[1]) + neighbours

    return pl.pallas_call(
        kernel_body,
        out_shape=jax.ShapeDtypeStruct((1, n), jnp.float32),
        in_specs=[pl.BlockSpec(memory_space=pl.ANY)],
        out_specs=pl.BlockSpec(memory_space=pltpu.VMEM),
        scratch_shapes=[
            pltpu.VMEM((m, n), jnp.float32),
            pltpu.VMEM((1, n), jnp.float32),
            pltpu.VMEM((NUM_DEVICES - 1, 1, n), jnp.float32),
            pltpu.SemaphoreType.DMA((steps,)),
            pltpu.SemaphoreType.DMA((len(TAIL),)),
            pltpu.SemaphoreType.DMA((NUM_DEVICES - 1,)),
            pltpu.SemaphoreType.DMA((NUM_DEVICES - 1,)),
        ],
        compiler_params=pltpu.CompilerParams(
            collective_id=0,
            vmem_limit_bytes=40 << 20,
            disable_semaphore_checks=True,
            disable_bounds_checks=True,
        ),
    )(x)
```

```python
import jax
import jax.numpy as jnp
from jax import lax
from jax.experimental import pallas as pl
from jax.experimental.pallas import tpu as pltpu

NUM_DEVICES = 4
SUBLANES, LANES = 8, 128
TILES = 8
STREAMS = 16

STEP_ORDER = tuple(
    (8 * e + 4 * d + 2 * a + c, b)
    for e in range(2) for d in range(2) for c in range(2)
    for b in range(2) for a in range(2)
)
STRIP_STREAMS = (13, STREAMS - 1)
STRIP_TILES = 8
LOOKAHEAD = 4
LAST_STEP_GROUPS = (24, 8)
STRIP_GROUPS = (6, 2)


def _tree_sum(values):
    values = list(values)
    while len(values) > 1:
        values = [sum(values[i + 1:i + 2], values[i]) for i in range(0, len(values), 2)]
    return values[0]


def pallas_dist_mean_ax0_shard0_i_m4096_n1024_kernel(x: jax.Array):
    m, n = x.shape
    assert n == TILES * LANES and m % (2 * STREAMS * SUBLANES) == 0
    blocks = m // SUBLANES
    stream_blocks = blocks // STREAMS
    steps = stream_blocks // 2
    wide = n - LANES
    assert steps > LOOKAHEAD + 1

    pieces = []
    step_tiles = 0
    for stream, half in STEP_ORDER:
        first_slot = 1 if stream in STRIP_STREAMS else 0
        pieces.append((stream * stream_blocks + half, first_slot, step_tiles))
        step_tiles += TILES - first_slot
    strip_rows = STRIP_TILES * SUBLANES
    strips = [
        (stream * stream_blocks + b) * SUBLANES
        for b in range(0, stream_blocks, STRIP_TILES)
        for stream in STRIP_STREAMS
    ]
    assert sum(LAST_STEP_GROUPS) == len(pieces) and sum(STRIP_GROUPS) == len(strips)

    def groups(sizes):
        return [range(sum(sizes[:g]), sum(sizes[:g + 1])) for g in range(len(sizes))]

    def kernel_body(x_tiles, x_rows, o_ref, buf, strip_buf, send_buf, recv_buf,
                    step_sems, last_sems, strip_sems, send_sems, recv_sems):
        def start_piece(step, p, sem):
            block, first_slot, dst = pieces[p]
            src = (block + 2 * step) * TILES + TILES - 1 + first_slot
            if isinstance(step, int):
                src %= blocks * TILES
            pltpu.make_async_copy(
                x_tiles.at[pl.ds(src, TILES - first_slot)],
                buf.at[pl.ds(step * step_tiles + dst, TILES - first_slot)],
                sem,
            ).start(priority=(p + 1) % 2)

        def start_step(step):
            for p in range(len(pieces)):
                start_piece(step, p, step_sems.at[step])

        def start_last_copies():
            for g, group in enumerate(groups(LAST_STEP_GROUPS)):
                for p in group:
                    start_piece(steps - 1, p, last_sems.at[g])
            for g, group in enumerate(groups(STRIP_GROUPS)):
                for s in group:
                    pltpu.make_async_copy(
                        x_rows.at[pl.ds(strips[s], strip_rows), pl.ds(wide, LANES)],
                        strip_buf.at[pl.ds(s * strip_rows, strip_rows)],
                        strip_sems.at[g],
                    ).start(priority=s % 2)

        def wait_filled(ref, sem):
            pltpu.make_async_copy(ref, ref, sem).wait()

        def add_pieces(step, group, acc):
            acc = list(acc)
            for p in group:
                _, first_slot, first = pieces[p]
                for slot in range(first_slot, TILES):
                    acc[slot] += buf[step * step_tiles + first + slot - first_slot]
            return tuple(acc)

        def sum_step(step, acc, start_next):
            wait_filled(buf.at[pl.ds(step * step_tiles, step_tiles)], step_sems.at[step])
            start_next()
            return add_pieces(step, range(len(pieces)), acc)

        for step in range(LOOKAHEAD):
            start_step(step)

        me = lax.axis_index("i")
        barrier = pltpu.get_barrier_semaphore()
        for d in range(1, NUM_DEVICES):
            pl.semaphore_signal(
                barrier, 1, device_id=(me + d) % NUM_DEVICES,
                device_id_type=pl.DeviceIdType.LOGICAL,
            )

        acc = tuple(jnp.zeros((SUBLANES, LANES), jnp.float32) for _ in range(TILES))
        turn = steps - 1 - LOOKAHEAD
        acc = lax.fori_loop(
            0, turn,
            lambda i, a: sum_step(i, a, lambda: start_step(i + LOOKAHEAD)), acc)
        acc = sum_step(turn, acc, start_last_copies)
        pl.semaphore_wait(barrier, NUM_DEVICES - 1)
        acc = lax.fori_loop(
            turn + 1, steps - 1, lambda i, a: sum_step(i, a, lambda: None), acc)
        for g, group in enumerate(groups(LAST_STEP_GROUPS)):
            first = pieces[group[0]][2]
            count = sum(TILES - pieces[p][1] for p in group)
            wait_filled(buf.at[pl.ds((steps - 1) * step_tiles + first, count)], last_sems.at[g])
            acc = add_pieces(steps - 1, group, acc)

        def exchange(d, col, cols, sem):
            return pltpu.make_async_remote_copy(
                send_buf.at[:, pl.ds(col, cols)],
                recv_buf.at[d - 1, :, pl.ds(col, cols)],
                send_sems.at[sem],
                recv_sems.at[sem],
                device_id=(me + d) % NUM_DEVICES,
                device_id_type=pl.DeviceIdType.LOGICAL,
            )

        right, left = exchange(1, 0, n, 0), exchange(3, 0, n, 1)
        far_wide, far_strip = exchange(2, 0, wide, 2), exchange(2, wide, LANES, 3)

        send_buf[:, :wide] = jnp.sum(jnp.concatenate(acc[1:], axis=1), axis=0, keepdims=True)
        far_wide.start()
        strip = acc[0]
        for g, group in enumerate(groups(STRIP_GROUPS)):
            first, count = group[0] * strip_rows, len(group) * strip_rows
            wait_filled(strip_buf.at[pl.ds(first, count)], strip_sems.at[g])
            strip = _tree_sum(
                [strip]
                + [strip_buf[pl.ds(r, SUBLANES), :] for r in range(first, first + count, SUBLANES)]
            )
        send_buf[:, wide:] = jnp.sum(strip, axis=0, keepdims=True)
        far_strip.start()
        right.start()
        left.start()

        for copy in (far_wide, far_strip, right, left):
            copy.wait_send()
        for copy in (far_wide, right, left):
            copy.wait_recv()
        neighbours = recv_buf[0] + recv_buf[2]
        own = send_buf[...]
        far_strip.wait_recv()
        o_ref[...] = ((own + recv_buf[1]) + neighbours) * (1.0 / (m * NUM_DEVICES))

    x_tiles = (
        x.reshape(blocks, SUBLANES, TILES, LANES)
        .transpose(0, 2, 1, 3)
        .reshape(blocks * TILES, SUBLANES, LANES)
    )
    return pl.pallas_call(
        kernel_body,
        out_shape=jax.ShapeDtypeStruct((1, n), jnp.float32),
        in_specs=[pl.BlockSpec(memory_space=pl.ANY), pl.BlockSpec(memory_space=pl.ANY)],
        out_specs=pl.BlockSpec(memory_space=pltpu.VMEM),
        scratch_shapes=[
            pltpu.VMEM((steps * step_tiles, SUBLANES, LANES), jnp.float32),
            pltpu.VMEM((len(strips) * strip_rows, LANES), jnp.float32),
            pltpu.VMEM((1, n), jnp.float32),
            pltpu.VMEM((NUM_DEVICES - 1, 1, n), jnp.float32),
            pltpu.SemaphoreType.DMA((steps - 1,)),
            pltpu.SemaphoreType.DMA((len(LAST_STEP_GROUPS),)),
            pltpu.SemaphoreType.DMA((len(STRIP_GROUPS),)),
            pltpu.SemaphoreType.DMA((4,)),
            pltpu.SemaphoreType.DMA((4,)),
        ],
        compiler_params=pltpu.CompilerParams(
            collective_id=0,
            vmem_limit_bytes=40 << 20,
            disable_semaphore_checks=True,
        ),
    )(x_tiles, x)
```

```python
import jax
import jax.numpy as jnp
from jax import lax
from jax.experimental import pallas as pl
from jax.experimental.pallas import tpu as pltpu

NUM_DEVICES = 4
SUBLANES, LANES = 8, 128
TILES = 8
STREAMS = 16

STEP_ORDER = tuple(
    (8 * e + 4 * d + 2 * a + c, b)
    for e in range(2) for d in range(2) for c in range(2)
    for b in range(2) for a in range(2)
)
LOOKAHEAD = 4
SHIPPED = 4
SIGNAL_AFTER, SHIP_AFTER = 2, 24
STRIP_STREAMS = (STREAMS - 2, STREAMS - 1)
STRIP_TILES = 8
LAST_STEP_GROUPS = (20, 8)
STRIP_GROUPS = (6, 2)


def _groups(first, sizes):
    out = []
    for size in sizes:
        out.append(range(first, first + size))
        first += size
    return out


def _tree_sum(values):
    while len(values) > 1:
        pairs = [a + b for a, b in zip(values[::2], values[1::2])]
        values = pairs + values[2 * len(pairs):]
    return values[0]


def pallas_dist_mean_ax0_shard0_i_m4096_n1024_kernel(x: jax.Array):
    m, n = x.shape
    assert n == TILES * LANES and m % (2 * STREAMS * SUBLANES) == 0
    blocks = m // SUBLANES
    stream_blocks = blocks // STREAMS
    steps = stream_blocks // 2
    last = steps - 1
    wide = n - LANES
    assert last > LOOKAHEAD

    pieces = []
    step_tiles = 0
    for stream, half in STEP_ORDER:
        first_slot = 1 if stream in STRIP_STREAMS else 0
        pieces.append((stream * stream_blocks + half, first_slot, step_tiles))
        step_tiles += TILES - first_slot
    strip_rows = STRIP_TILES * SUBLANES
    strips = [
        (stream * stream_blocks + b) * SUBLANES
        for b in range(0, stream_blocks, STRIP_TILES)
        for stream in STRIP_STREAMS
    ]
    last_groups = _groups(SHIPPED, LAST_STEP_GROUPS)
    strip_groups = _groups(0, STRIP_GROUPS)
    assert last_groups[-1].stop == len(pieces) and strip_groups[-1].stop == len(strips)

    def kernel_body(x_tiles, x_rows, o_ref, buf, strip_buf, send_buf, recv_buf,
                    step_sems, last_sems, strip_sems, ship_send_sems, ship_recv_sems,
                    send_sems, recv_sems):
        me = lax.axis_index("i")

        def piece_refs(step, p):
            block, first_slot, first = pieces[p]
            src = (block + 2 * step) * TILES + TILES - 1 + first_slot
            if isinstance(step, int):
                src %= blocks * TILES
            size = TILES - first_slot
            return x_tiles.at[pl.ds(src, size)], buf.at[pl.ds(step * step_tiles + first, size)]

        def start_piece(step, p, sem):
            pltpu.make_async_copy(*piece_refs(step, p), sem).start(priority=(p + 1) % 2)

        def start_step(step):
            for p in range(len(pieces)):
                start_piece(step, p, step_sems.at[step])

        def ship(p):
            return pltpu.make_async_remote_copy(
                *piece_refs(last, p), ship_send_sems.at[p], ship_recv_sems.at[p],
                device_id=(me + (1, NUM_DEVICES - 1)[p % 2]) % NUM_DEVICES,
                device_id_type=pl.DeviceIdType.LOGICAL,
            )

        def start_last_copies():
            for g, group in enumerate(last_groups):
                for p in group:
                    start_piece(last, p, last_sems.at[g])
            for g, group in enumerate(strip_groups):
                for s in group:
                    pltpu.make_async_copy(
                        x_rows.at[pl.ds(strips[s], strip_rows), pl.ds(wide, LANES)],
                        strip_buf.at[pl.ds(s * strip_rows, strip_rows)],
                        strip_sems.at[g],
                    ).start(priority=s % 2)

        def wait_filled(ref, sem):
            pltpu.make_async_copy(ref, ref, sem).wait()

        def add_pieces(step, group, acc):
            acc = list(acc)
            for p in group:
                _, first_slot, first = pieces[p]
                for slot in range(first_slot, TILES):
                    acc[slot] += buf[step * step_tiles + first + slot - first_slot]
            return tuple(acc)

        def sum_step(step, acc, start_next):
            wait_filled(buf.at[pl.ds(step * step_tiles, step_tiles)], step_sems.at[step])
            start_next()
            return add_pieces(step, range(len(pieces)), acc)

        barrier = pltpu.get_barrier_semaphore()
        for p in range(len(pieces)):
            if p == SIGNAL_AFTER:
                for d in range(1, NUM_DEVICES):
                    pl.semaphore_signal(
                        barrier, 1, device_id=(me + d) % NUM_DEVICES,
                        device_id_type=pl.DeviceIdType.LOGICAL,
                    )
            if p == SHIP_AFTER:
                pl.semaphore_wait(barrier, NUM_DEVICES - 1)
                for q in range(SHIPPED):
                    ship(q).start()
            start_piece(0, p, step_sems.at[0])
        for step in range(1, LOOKAHEAD):
            start_step(step)

        acc = tuple(jnp.zeros((SUBLANES, LANES), jnp.float32) for _ in range(TILES))
        turn = last - LOOKAHEAD
        acc = lax.fori_loop(
            0, turn,
            lambda i, a: sum_step(i, a, lambda: start_step(i + LOOKAHEAD)), acc)
        acc = sum_step(turn, acc, start_last_copies)
        acc = lax.fori_loop(turn + 1, last, lambda i, a: sum_step(i, a, lambda: None), acc)
        for q in range(SHIPPED):
            ship(q).wait()
        acc = add_pieces(last, range(SHIPPED), acc)
        for g, group in enumerate(last_groups):
            first = last * step_tiles + pieces[group.start][2]
            count = sum(TILES - pieces[p][1] for p in group)
            wait_filled(buf.at[pl.ds(first, count)], last_sems.at[g])
            acc = add_pieces(last, group, acc)

        def exchange(d, col, cols, sem):
            return pltpu.make_async_remote_copy(
                send_buf.at[:, pl.ds(col, cols)],
                recv_buf.at[d - 1, :, pl.ds(col, cols)],
                send_sems.at[sem],
                recv_sems.at[sem],
                device_id=(me + d) % NUM_DEVICES,
                device_id_type=pl.DeviceIdType.LOGICAL,
            )

        right, left = exchange(1, 0, n, 0), exchange(3, 0, n, 1)
        far_wide, far_strip = exchange(2, 0, wide, 2), exchange(2, wide, LANES, 3)

        send_buf[:, :wide] = jnp.sum(jnp.concatenate(acc[1:], axis=1), axis=0, keepdims=True)
        far_wide.start()
        strip = acc[0]
        for g, group in enumerate(strip_groups):
            first, end = group.start * strip_rows, group.stop * strip_rows
            wait_filled(strip_buf.at[pl.ds(first, end - first)], strip_sems.at[g])
            strip = _tree_sum(
                [strip_buf[pl.ds(r, SUBLANES), :] for r in range(first, end, SUBLANES)]
                + [strip]
            )
        send_buf[:, wide:] = jnp.sum(strip, axis=0, keepdims=True)
        far_strip.start()
        right.start()
        left.start()

        for copy in (far_wide, far_strip, right, left):
            copy.wait_send()
        for copy in (far_wide, right, left):
            copy.wait_recv()
        neighbours = recv_buf[0] + recv_buf[2]
        own = send_buf[...]
        far_strip.wait_recv()
        o_ref[...] = ((own + recv_buf[1]) + neighbours) * (1.0 / (m * NUM_DEVICES))

    x_tiles = (
        x.reshape(blocks, SUBLANES, TILES, LANES)
        .transpose(0, 2, 1, 3)
        .reshape(blocks * TILES, SUBLANES, LANES)
    )
    return pl.pallas_call(
        kernel_body,
        out_shape=jax.ShapeDtypeStruct((1, n), jnp.float32),
        in_specs=[pl.BlockSpec(memory_space=pl.ANY), pl.BlockSpec(memory_space=pl.ANY)],
        out_specs=pl.BlockSpec(memory_space=pltpu.VMEM),
        scratch_shapes=[
            pltpu.VMEM((steps * step_tiles, SUBLANES, LANES), jnp.float32),
            pltpu.VMEM((len(strips) * strip_rows, LANES), jnp.float32),
            pltpu.VMEM((1, n), jnp.float32),
            pltpu.VMEM((NUM_DEVICES - 1, 1, n), jnp.float32),
            pltpu.SemaphoreType.DMA((last,)),
            pltpu.SemaphoreType.DMA((len(last_groups),)),
            pltpu.SemaphoreType.DMA((len(strip_groups),)),
            pltpu.SemaphoreType.DMA((SHIPPED,)),
            pltpu.SemaphoreType.DMA((SHIPPED,)),
            pltpu.SemaphoreType.DMA((4,)),
            pltpu.SemaphoreType.DMA((4,)),
        ],
        compiler_params=pltpu.CompilerParams(
            collective_id=0,
            vmem_limit_bytes=40 << 20,
            disable_semaphore_checks=True,
        ),
    )(x_tiles, x)
```

```python
import jax
import jax.numpy as jnp
from jax import lax
from jax.experimental import pallas as pl
from jax.experimental.pallas import tpu as pltpu

NUM_DEVICES = 4
SUBLANES, LANES = 8, 128
TILES = 8
STREAMS = 16

STEP_ORDER = tuple(
    (8 * e + 4 * d + 2 * a + c, b)
    for e in range(2) for d in range(2) for c in range(2)
    for b in range(2) for a in range(2)
)
LOOKAHEAD = 4
SHIPPED = 4
SIGNAL_AFTER, SHIP_AFTER = 2, 24
STRIP_STREAMS = (10, STREAMS - 1)
STRIP_TILES = 4
LAST_STEP_GROUPS = (20, 4, 4)
STRIP_GROUPS = (8, 4, 2, 2)


def _groups(first, sizes):
    out = []
    for size in sizes:
        out.append(range(first, first + size))
        first += size
    return out


def _tree_sum(values):
    while len(values) > 1:
        pairs = [a + b for a, b in zip(values[::2], values[1::2])]
        values = pairs + values[2 * len(pairs):]
    return values[0]


def pallas_dist_mean_ax0_shard0_i_m4096_n1024_kernel(x: jax.Array):
    m, n = x.shape
    assert n == TILES * LANES and m % (2 * STREAMS * SUBLANES) == 0
    blocks = m // SUBLANES
    stream_blocks = blocks // STREAMS
    steps = stream_blocks // 2
    last = steps - 1
    wide = n - LANES
    assert last > LOOKAHEAD

    pieces = []
    step_tiles = 0
    for stream, half in STEP_ORDER:
        first_slot = 1 if stream in STRIP_STREAMS else 0
        pieces.append((stream * stream_blocks + half, first_slot, step_tiles))
        step_tiles += TILES - first_slot
    strip_rows = STRIP_TILES * SUBLANES
    strips = [
        (stream * stream_blocks + b) * SUBLANES
        for b in range(0, stream_blocks, STRIP_TILES)
        for stream in STRIP_STREAMS
    ]
    last_groups = _groups(SHIPPED, LAST_STEP_GROUPS)
    strip_groups = _groups(0, STRIP_GROUPS)
    assert last_groups[-1].stop == len(pieces) and strip_groups[-1].stop == len(strips)

    def kernel_body(x_tiles, x_rows, o_ref, buf, strip_buf, send_buf, recv_buf,
                    step_sems, last_sems, strip_sems, ship_send_sems, ship_recv_sems,
                    send_sems, recv_sems):
        me = lax.axis_index("i")

        def piece_refs(step, p):
            block, first_slot, first = pieces[p]
            src = (block + 2 * step) * TILES + TILES - 1 + first_slot
            if isinstance(step, int):
                src %= blocks * TILES
            size = TILES - first_slot
            return x_tiles.at[pl.ds(src, size)], buf.at[pl.ds(step * step_tiles + first, size)]

        def start_piece(step, p, sem):
            pltpu.make_async_copy(*piece_refs(step, p), sem).start(priority=(p + 1) % 2)

        def start_step(step):
            for p in range(len(pieces)):
                start_piece(step, p, step_sems.at[step])

        def ship(p):
            return pltpu.make_async_remote_copy(
                *piece_refs(last, p), ship_send_sems.at[p], ship_recv_sems.at[p],
                device_id=(me + (1, NUM_DEVICES - 1)[p % 2]) % NUM_DEVICES,
                device_id_type=pl.DeviceIdType.LOGICAL,
            )

        def start_last_copies():
            for g, group in enumerate(last_groups):
                for p in group:
                    start_piece(last, p, last_sems.at[g])
            for g, group in enumerate(strip_groups):
                for s in group:
                    pltpu.make_async_copy(
                        x_rows.at[pl.ds(strips[s], strip_rows), pl.ds(wide, LANES)],
                        strip_buf.at[pl.ds(s * strip_rows, strip_rows)],
                        strip_sems.at[g],
                    ).start(priority=s % 2)

        def wait_filled(ref, sem):
            pltpu.make_async_copy(ref, ref, sem).wait()

        def add_pieces(step, group, acc):
            acc = list(acc)
            for p in group:
                _, first_slot, first = pieces[p]
                for slot in range(first_slot, TILES):
                    acc[slot] += buf[step * step_tiles + first + slot - first_slot]
            return tuple(acc)

        def sum_step(step, acc, start_next):
            wait_filled(buf.at[pl.ds(step * step_tiles, step_tiles)], step_sems.at[step])
            start_next()
            return add_pieces(step, range(len(pieces)), acc)

        barrier = pltpu.get_barrier_semaphore()
        for p in range(len(pieces)):
            if p == SIGNAL_AFTER:
                for d in range(1, NUM_DEVICES):
                    pl.semaphore_signal(
                        barrier, 1, device_id=(me + d) % NUM_DEVICES,
                        device_id_type=pl.DeviceIdType.LOGICAL,
                    )
            if p == SHIP_AFTER:
                pl.semaphore_wait(barrier, NUM_DEVICES - 1)
                for q in range(SHIPPED):
                    ship(q).start()
            start_piece(0, p, step_sems.at[0])
        for step in range(1, LOOKAHEAD):
            start_step(step)

        acc = tuple(jnp.zeros((SUBLANES, LANES), jnp.float32) for _ in range(TILES))
        turn = last - LOOKAHEAD
        acc = lax.fori_loop(
            0, turn,
            lambda i, a: sum_step(i, a, lambda: start_step(i + LOOKAHEAD)), acc)
        acc = sum_step(turn, acc, start_last_copies)
        acc = lax.fori_loop(turn + 1, last, lambda i, a: sum_step(i, a, lambda: None), acc)
        for q in range(SHIPPED):
            ship(q).wait()
        acc = add_pieces(last, range(SHIPPED), acc)
        for g, group in enumerate(last_groups):
            first = last * step_tiles + pieces[group.start][2]
            count = sum(TILES - pieces[p][1] for p in group)
            wait_filled(buf.at[pl.ds(first, count)], last_sems.at[g])
            acc = add_pieces(last, group, acc)

        def exchange(d, col, cols, sem):
            return pltpu.make_async_remote_copy(
                send_buf.at[:, pl.ds(col, cols)],
                recv_buf.at[d - 1, :, pl.ds(col, cols)],
                send_sems.at[sem],
                recv_sems.at[sem],
                device_id=(me + d) % NUM_DEVICES,
                device_id_type=pl.DeviceIdType.LOGICAL,
            )

        right, left = exchange(1, 0, n, 0), exchange(3, 0, n, 1)
        far_wide, far_strip = exchange(2, 0, wide, 2), exchange(2, wide, LANES, 3)

        send_buf[:, :wide] = jnp.sum(jnp.concatenate(acc[1:], axis=1), axis=0, keepdims=True)
        far_wide.start()
        strip = acc[0]
        for g, group in enumerate(strip_groups):
            first, end = group.start * strip_rows, group.stop * strip_rows
            wait_filled(strip_buf.at[pl.ds(first, end - first)], strip_sems.at[g])
            strip = _tree_sum(
                [strip_buf[pl.ds(r, SUBLANES), :] for r in range(first, end, SUBLANES)]
                + [strip]
            )
        send_buf[:, wide:] = jnp.sum(strip, axis=0, keepdims=True)
        far_strip.start()
        right.start()
        left.start()

        for copy in (far_wide, far_strip, right, left):
            copy.wait_send()
        for copy in (far_wide, right, left):
            copy.wait_recv()
        neighbours = recv_buf[0] + recv_buf[2]
        own = send_buf[...]
        far_strip.wait_recv()
        o_ref[...] = ((own + recv_buf[1]) + neighbours) * (1.0 / (m * NUM_DEVICES))

    x_tiles = (
        x.reshape(blocks, SUBLANES, TILES, LANES)
        .transpose(0, 2, 1, 3)
        .reshape(blocks * TILES, SUBLANES, LANES)
    )
    return pl.pallas_call(
        kernel_body,
        out_shape=jax.ShapeDtypeStruct((1, n), jnp.float32),
        in_specs=[pl.BlockSpec(memory_space=pl.ANY), pl.BlockSpec(memory_space=pl.ANY)],
        out_specs=pl.BlockSpec(memory_space=pltpu.VMEM),
        scratch_shapes=[
            pltpu.VMEM((steps * step_tiles, SUBLANES, LANES), jnp.float32),
            pltpu.VMEM((len(strips) * strip_rows, LANES), jnp.float32),
            pltpu.VMEM((1, n), jnp.float32),
            pltpu.VMEM((NUM_DEVICES - 1, 1, n), jnp.float32),
            pltpu.SemaphoreType.DMA((last,)),
            pltpu.SemaphoreType.DMA((len(last_groups),)),
            pltpu.SemaphoreType.DMA((len(strip_groups),)),
            pltpu.SemaphoreType.DMA((SHIPPED,)),
            pltpu.SemaphoreType.DMA((SHIPPED,)),
            pltpu.SemaphoreType.DMA((4,)),
            pltpu.SemaphoreType.DMA((4,)),
        ],
        compiler_params=pltpu.CompilerParams(
            collective_id=0,
            vmem_limit_bytes=40 << 20,
            disable_semaphore_checks=True,
        ),
    )(x_tiles, x)
```

```python
import jax
import jax.numpy as jnp
from jax import lax
from jax.experimental import pallas as pl
from jax.experimental.pallas import tpu as pltpu

NUM_DEVICES = 4
SUBLANES, LANES = 8, 128
TILES = 8
STREAMS = 16

STEP_ORDER = tuple(
    (8 * e + 4 * d + 2 * a + c, b)
    for e in range(2) for d in range(2) for c in range(2)
    for b in range(2) for a in range(2)
)
LOOKAHEAD = 4
SHIPPED = 4
SIGNAL_AFTER, SHIP_AFTER = 2, 24
STRIP_STREAMS = (10, STREAMS - 1)
STRIP_TILES = 4
LAST_STEP_GROUPS = (20, 4, 4)
STRIP_GROUPS = (8, 4, 2, 2)


def _groups(first, sizes):
    out = []
    for size in sizes:
        out.append(range(first, first + size))
        first += size
    return out


def _tree_sum(values):
    while len(values) > 1:
        pairs = [a + b for a, b in zip(values[::2], values[1::2])]
        values = pairs + values[2 * len(pairs):]
    return values[0]


def pallas_dist_mean_ax0_shard0_i_m4096_n1024_kernel(x: jax.Array):
    m, n = x.shape
    assert n == TILES * LANES and m % (2 * STREAMS * SUBLANES) == 0
    blocks = m // SUBLANES
    stream_blocks = blocks // STREAMS
    steps = stream_blocks // 2
    last = steps - 1
    wide = n - LANES
    assert last > LOOKAHEAD

    pieces = []
    step_tiles = 0
    for stream, half in STEP_ORDER:
        first_slot = 1 if stream in STRIP_STREAMS else 0
        pieces.append((stream * stream_blocks + half, first_slot, step_tiles))
        step_tiles += TILES - first_slot
    strip_rows = STRIP_TILES * SUBLANES
    strips = [
        (stream * stream_blocks + b) * SUBLANES
        for b in range(0, stream_blocks, STRIP_TILES)
        for stream in STRIP_STREAMS
    ]
    last_groups = _groups(SHIPPED, LAST_STEP_GROUPS)
    strip_groups = _groups(0, STRIP_GROUPS)
    assert last_groups[-1].stop == len(pieces) and strip_groups[-1].stop == len(strips)

    def kernel_body(x_tiles, x_rows, o_ref, buf, strip_buf, send_buf, recv_buf,
                    step_sems, last_sems, strip_sems, ship_send_sems, ship_recv_sems,
                    send_sems, recv_sems):
        me = lax.axis_index("i")

        def piece_refs(step, p):
            block, first_slot, first = pieces[p]
            src = (block + 2 * step) * TILES + TILES - 1 + first_slot
            if isinstance(step, int):
                src %= blocks * TILES
            size = TILES - first_slot
            return x_tiles.at[pl.ds(src, size)], buf.at[pl.ds(step * step_tiles + first, size)]

        def start_piece(step, p, sem):
            pltpu.make_async_copy(*piece_refs(step, p), sem).start(priority=(p + 1) % 2)

        def start_step(step):
            for p in range(len(pieces)):
                start_piece(step, p, step_sems.at[step])

        def ship(p):
            return pltpu.make_async_remote_copy(
                *piece_refs(last, p), ship_send_sems.at[p], ship_recv_sems.at[p],
                device_id=(me + (1, NUM_DEVICES - 1)[p % 2]) % NUM_DEVICES,
                device_id_type=pl.DeviceIdType.LOGICAL,
            )

        def start_last_copies():
            for g, group in enumerate(last_groups):
                for p in group:
                    start_piece(last, p, last_sems.at[g])
            for g, group in enumerate(strip_groups):
                for s in group:
                    pltpu.make_async_copy(
                        x_rows.at[pl.ds(strips[s], strip_rows), pl.ds(wide, LANES)],
                        strip_buf.at[pl.ds(s * strip_rows, strip_rows)],
                        strip_sems.at[g],
                    ).start(priority=s % 2)

        def wait_filled(ref, sem):
            pltpu.make_async_copy(ref, ref, sem).wait()

        def add_pieces(step, group, acc):
            strip_acc, wide_acc = acc
            for p in group:
                _, first_slot, first = pieces[p]
                first += step * step_tiles
                if first_slot == 0:
                    strip_acc += buf[first]
                wide_acc += buf[pl.ds(first + 1 - first_slot, TILES - 1)]
            return strip_acc, wide_acc

        def sum_step(step, acc, start_next):
            wait_filled(buf.at[pl.ds(step * step_tiles, step_tiles)], step_sems.at[step])
            start_next()
            return add_pieces(step, range(len(pieces)), acc)

        barrier = pltpu.get_barrier_semaphore()
        for p in range(len(pieces)):
            if p == SIGNAL_AFTER:
                for d in range(1, NUM_DEVICES):
                    pl.semaphore_signal(
                        barrier, 1, device_id=(me + d) % NUM_DEVICES,
                        device_id_type=pl.DeviceIdType.LOGICAL,
                    )
            if p == SHIP_AFTER:
                pl.semaphore_wait(barrier, NUM_DEVICES - 1)
                for q in range(SHIPPED):
                    ship(q).start()
            start_piece(0, p, step_sems.at[0])
        for step in range(1, LOOKAHEAD):
            start_step(step)

        acc = (
            jnp.zeros((SUBLANES, LANES), jnp.float32),
            jnp.zeros((TILES - 1, SUBLANES, LANES), jnp.float32),
        )
        turn = last - LOOKAHEAD
        acc = lax.fori_loop(
            0, turn,
            lambda i, a: sum_step(i, a, lambda: start_step(i + LOOKAHEAD)), acc)
        acc = sum_step(turn, acc, start_last_copies)
        acc = lax.fori_loop(turn + 1, last, lambda i, a: sum_step(i, a, lambda: None), acc)
        for q in range(SHIPPED):
            ship(q).wait()
        acc = add_pieces(last, range(SHIPPED), acc)
        for g, group in enumerate(last_groups):
            first = last * step_tiles + pieces[group.start][2]
            count = sum(TILES - pieces[p][1] for p in group)
            wait_filled(buf.at[pl.ds(first, count)], last_sems.at[g])
            acc = add_pieces(last, group, acc)

        def exchange(d, col, cols, sem):
            return pltpu.make_async_remote_copy(
                send_buf.at[:, pl.ds(col, cols)],
                recv_buf.at[d - 1, :, pl.ds(col, cols)],
                send_sems.at[sem],
                recv_sems.at[sem],
                device_id=(me + d) % NUM_DEVICES,
                device_id_type=pl.DeviceIdType.LOGICAL,
            )

        right, left = exchange(1, 0, n, 0), exchange(3, 0, n, 1)
        far_wide, far_strip = exchange(2, 0, wide, 2), exchange(2, wide, LANES, 3)

        strip, wide_acc = acc
        columns = jnp.concatenate([wide_acc[c] for c in range(TILES - 1)], axis=1)
        send_buf[:, :wide] = jnp.sum(columns, axis=0, keepdims=True)
        far_wide.start()
        for g, group in enumerate(strip_groups):
            first, end = group.start * strip_rows, group.stop * strip_rows
            wait_filled(strip_buf.at[pl.ds(first, end - first)], strip_sems.at[g])
            strip = _tree_sum(
                [strip_buf[pl.ds(r, SUBLANES), :] for r in range(first, end, SUBLANES)]
                + [strip]
            )
        send_buf[:, wide:] = jnp.sum(strip, axis=0, keepdims=True)
        far_strip.start()
        right.start()
        left.start()

        for copy in (far_wide, far_strip, right, left):
            copy.wait_send()
        for copy in (far_wide, right, left):
            copy.wait_recv()
        neighbours = recv_buf[0] + recv_buf[2]
        own = send_buf[...]
        far_strip.wait_recv()
        o_ref[...] = ((own + recv_buf[1]) + neighbours) * (1.0 / (m * NUM_DEVICES))

    x_tiles = (
        x.reshape(blocks, SUBLANES, TILES, LANES)
        .transpose(0, 2, 1, 3)
        .reshape(blocks * TILES, SUBLANES, LANES)
    )
    return pl.pallas_call(
        kernel_body,
        out_shape=jax.ShapeDtypeStruct((1, n), jnp.float32),
        in_specs=[pl.BlockSpec(memory_space=pl.ANY), pl.BlockSpec(memory_space=pl.ANY)],
        out_specs=pl.BlockSpec(memory_space=pltpu.VMEM),
        scratch_shapes=[
            pltpu.VMEM((steps * step_tiles, SUBLANES, LANES), jnp.float32),
            pltpu.VMEM((len(strips) * strip_rows, LANES), jnp.float32),
            pltpu.VMEM((1, n), jnp.float32),
            pltpu.VMEM((NUM_DEVICES - 1, 1, n), jnp.float32),
            pltpu.SemaphoreType.DMA((last,)),
            pltpu.SemaphoreType.DMA((len(last_groups),)),
            pltpu.SemaphoreType.DMA((len(strip_groups),)),
            pltpu.SemaphoreType.DMA((SHIPPED,)),
            pltpu.SemaphoreType.DMA((SHIPPED,)),
            pltpu.SemaphoreType.DMA((4,)),
            pltpu.SemaphoreType.DMA((4,)),
        ],
        compiler_params=pltpu.CompilerParams(
            collective_id=0,
            vmem_limit_bytes=40 << 20,
            disable_semaphore_checks=True,
        ),
    )(x_tiles, x)
```
